```python
import numpy as np

kernel_name = "dist_mean_ax0_shard0_i_m2048_n1024"

def setup_inputs():
    return {"x": np.random.randn(8192, 1024).astype(np.float32)}

def reference(x: np.ndarray) -> np.ndarray:
    return np.mean(x, axis=0, keepdims=True)
```

```python
import jax
import jax.numpy as jnp
from jax import lax
from jax.experimental import pallas as pl
from jax.experimental.pallas import tpu as pltpu

N_DEV = 4
SUBLANES = 8
STREAMS = 8
AHEAD = 16
TAIL = (4, 2, 2)


def _tree_sum(vals):
    while len(vals) > 1:
        pairs = [vals[i] + vals[i + 1] for i in range(0, len(vals) - 1, 2)]
        vals = pairs + ([vals[-1]] if len(vals) % 2 else [])
    return vals[0]


def pallas_dist_mean_ax0_shard0_i_m2048_n1024_kernel(
    x: jax.Array,
):
    m, n = x.shape
    groups = m // (SUBLANES * STREAMS)
    scale = 1.0 / (m * N_DEV)
    tail_starts = [sum(TAIL[:i]) for i in range(len(TAIL))]

    def kernel_body(x_hbm, o_ref, buf, stage, comm, in_sems, tail_sems, send_sem, nbr_sem, diag_sem):
        def fetch(g):
            for s in range(STREAMS):
                pltpu.make_async_copy(x_hbm.at[s, g], buf.at[g, s], in_sems.at[g]).start(priority=s % 2)

        def consume(g, acc):
            pltpu.make_async_copy(buf.at[g], buf.at[g], in_sems.at[g]).wait()
            return acc + _tree_sum([buf[g, s] for s in range(STREAMS)])

        def steady(g, acc):
            fetch(g + AHEAD)
            return consume(g, acc)

        lax.fori_loop(0, AHEAD, lambda g, _: fetch(g), None)
        me = lax.axis_index("i")
        barrier = pltpu.get_barrier_semaphore()
        for d in (2, 1, 3):
            pl.semaphore_signal(barrier, inc=1, device_id=(me ^ d,))

        last = groups - 1
        acc = lax.fori_loop(0, last - AHEAD, steady, jnp.zeros((SUBLANES, n), jnp.float32))
        for t, (s0, c) in enumerate(zip(tail_starts, TAIL)):
            for s in range(s0, s0 + c):
                pltpu.make_async_copy(x_hbm.at[s, last], buf.at[last, s], tail_sems.at[t]).start(priority=s % 2)
        pl.semaphore_wait(barrier, N_DEV - 1)
        acc = lax.fori_loop(last - AHEAD, last, consume, acc)
        for t, (s0, c) in enumerate(zip(tail_starts, TAIL)):
            piece = buf.at[last, pl.ds(s0, c)]
            pltpu.make_async_copy(piece, piece, tail_sems.at[t]).wait()
            acc = acc + _tree_sum([buf[last, s] for s in range(s0, s0 + c)])

        stage[...] = jnp.sum(acc, axis=0, keepdims=True)
        for d, slot, sem in ((2, 2, diag_sem), (1, 0, nbr_sem), (3, 1, nbr_sem)):
            pltpu.make_async_remote_copy(
                src_ref=stage, dst_ref=comm.at[slot], send_sem=send_sem, recv_sem=sem,
                device_id=(me ^ d,)).start()
        pltpu.make_async_copy(comm, comm, send_sem).wait()
        nbrs = comm.at[pl.ds(0, 2)]
        pltpu.make_async_copy(nbrs, nbrs, nbr_sem).wait()
        a = stage[...] + comm[0]
        b = comm[1]
        pltpu.make_async_copy(comm.at[2], comm.at[2], diag_sem).wait()
        o_ref[...] = (a + (b + comm[2])) * scale

    return pl.pallas_call(
        kernel_body,
        out_shape=jax.ShapeDtypeStruct((1, n), jnp.float32),
        in_specs=[pl.BlockSpec(memory_space=pltpu.HBM)],
        out_specs=pl.BlockSpec(memory_space=pltpu.VMEM),
        scratch_shapes=[
            pltpu.VMEM((groups, STREAMS, SUBLANES, n), jnp.float32),
            pltpu.VMEM((1, n), jnp.float32),
            pltpu.VMEM((N_DEV - 1, 1, n), jnp.float32),
            pltpu.SemaphoreType.DMA((groups - 1,)),
            pltpu.SemaphoreType.DMA((len(TAIL),)),
            pltpu.SemaphoreType.DMA,
            pltpu.SemaphoreType.DMA,
            pltpu.SemaphoreType.DMA,
        ],
        compiler_params=pltpu.CompilerParams(
            collective_id=0, disable_semaphore_checks=True, disable_bounds_checks=True),
    )(pltpu.with_memory_space_constraint(x.reshape(STREAMS, groups, SUBLANES, n), pltpu.HBM))
```

```python
import jax
import jax.numpy as jnp
from jax import lax
from jax.experimental import pallas as pl
from jax.experimental.pallas import tpu as pltpu

N_DEV = 4
ROWS = 8
STREAMS = 8
AHEAD = 16
LATE_GROUPS = 10
LATE_COLS = 128

DIAGONAL, NEIGHBOUR_A, NEIGHBOUR_B = 2, 1, 3


def _priority(stream):
    return 1 - stream % 2


def _tree_sum(vals):
    while len(vals) > 1:
        pairs = [vals[i] + vals[i + 1] for i in range(0, len(vals) - 1, 2)]
        vals = pairs + ([vals[-1]] if len(vals) % 2 else [])
    return vals[0]


def pallas_dist_mean_ax0_shard0_i_m2048_n1024_kernel(
    x: jax.Array,
):
    m, n = x.shape
    assert m % (ROWS * STREAMS) == 0 and n % LATE_COLS == 0
    stream_rows = m // STREAMS
    full_groups = stream_rows // ROWS - LATE_GROUPS
    assert full_groups >= AHEAD
    n_early = n - LATE_COLS
    early, late, every = pl.ds(0, n_early), pl.ds(n_early, LATE_COLS), pl.ds(0, n)

    def kernel_body(
        x_hbm, o_ref,
        full_buf, early_buf, late_buf, mine, theirs,
        full_sems, early_sems, late_sems, send_sems, recv_sems,
    ):
        def fetch(first_group, cols, buf, sems, g):
            for s in range(STREAMS):
                row = pl.multiple_of(s * stream_rows + (first_group + g) * ROWS, ROWS)
                pltpu.make_async_copy(
                    x_hbm.at[pl.ds(row, ROWS), cols], buf.at[g, s], sems.at[g]
                ).start(priority=_priority(s))

        def add_group(buf, sems, g, acc):
            pltpu.make_async_copy(buf.at[g], buf.at[g], sems.at[g]).wait()
            return acc + _tree_sum([buf[g, s] for s in range(STREAMS)])

        def fetch_full(g, carry=None):
            fetch(0, every, full_buf, full_sems, g)

        def add_full(g, acc):
            return add_group(full_buf, full_sems, g, acc)

        def fetch_and_add_full(g, acc):
            fetch_full(g + AHEAD)
            return add_full(g, acc)

        def send(i, peer, cols):
            return pltpu.make_async_remote_copy(
                src_ref=mine.at[:, cols],
                dst_ref=theirs.at[peer - 1, :, cols],
                send_sem=send_sems.at[i],
                recv_sem=recv_sems.at[i],
                device_id=(me ^ peer,),
                device_id_type=pl.DeviceIdType.MESH,
            )

        lax.fori_loop(0, AHEAD, fetch_full, None)

        me = lax.axis_index("i")
        barrier = pltpu.get_barrier_semaphore()
        for peer in (DIAGONAL, NEIGHBOUR_A, NEIGHBOUR_B):
            pl.semaphore_signal(
                barrier, inc=1, device_id=(me ^ peer,),
                device_id_type=pl.DeviceIdType.MESH,
            )

        acc = jnp.zeros((ROWS, n), jnp.float32)
        acc = lax.fori_loop(0, full_groups - AHEAD, fetch_and_add_full, acc)
        lax.fori_loop(
            0, LATE_GROUPS,
            lambda g, _: fetch(full_groups, early, early_buf, early_sems, g), None,
        )
        late_copies = []
        for s in range(STREAMS):
            rows = pl.ds(s * stream_rows + full_groups * ROWS, LATE_GROUPS * ROWS)
            late_copies.append(
                pltpu.make_async_copy(x_hbm.at[rows, late], late_buf.at[s], late_sems.at[s])
            )
            late_copies[s].start(priority=_priority(s))

        pl.semaphore_wait(barrier, N_DEV - 1)

        acc = lax.fori_loop(full_groups - AHEAD, full_groups, add_full, acc)
        early_acc = lax.fori_loop(
            0, LATE_GROUPS,
            lambda g, a: add_group(early_buf, early_sems, g, a), acc[:, :n_early],
        )
        mine[:, early] = jnp.sum(early_acc, axis=0, keepdims=True)
        diagonal_early = send(0, DIAGONAL, early)
        diagonal_early.start()

        late_acc = acc[:, n_early:]
        for s in sorted(range(STREAMS), key=_priority):
            late_copies[s].wait()
            late_acc = late_acc + _tree_sum(
                [late_buf[s, pl.ds(g * ROWS, ROWS), :] for g in range(LATE_GROUPS)]
            )
        mine[:, late] = jnp.sum(late_acc, axis=0, keepdims=True)
        diagonal_late = send(1, DIAGONAL, late)
        neighbour_a = send(2, NEIGHBOUR_A, every)
        neighbour_b = send(3, NEIGHBOUR_B, every)
        diagonal_late.start()
        neighbour_a.start()
        neighbour_b.start()

        for copy in (diagonal_early, diagonal_late, neighbour_a, neighbour_b):
            copy.wait_send()
        neighbour_a.wait_recv()
        neighbour_b.wait_recv()
        near = mine[...] + theirs[NEIGHBOUR_A - 1]
        other = theirs[NEIGHBOUR_B - 1]
        diagonal_early.wait_recv()
        diagonal_late.wait_recv()
        far = other + theirs[DIAGONAL - 1]
        o_ref[...] = (near + far) * (1.0 / (m * N_DEV))

    return pl.pallas_call(
        kernel_body,
        out_shape=jax.ShapeDtypeStruct((1, n), jnp.float32),
        in_specs=[pl.BlockSpec(memory_space=pltpu.HBM)],
        out_specs=pl.BlockSpec(memory_space=pltpu.VMEM),
        scratch_shapes=[
            pltpu.VMEM((full_groups, STREAMS, ROWS, n), jnp.float32),
            pltpu.VMEM((LATE_GROUPS, STREAMS, ROWS, n_early), jnp.float32),
            pltpu.VMEM((STREAMS, LATE_GROUPS * ROWS, LATE_COLS), jnp.float32),
            pltpu.VMEM((1, n), jnp.float32),
            pltpu.VMEM((N_DEV - 1, 1, n), jnp.float32),
            pltpu.SemaphoreType.DMA((full_groups,)),
            pltpu.SemaphoreType.DMA((LATE_GROUPS,)),
            pltpu.SemaphoreType.DMA((STREAMS,)),
            pltpu.SemaphoreType.DMA((4,)),
            pltpu.SemaphoreType.DMA((4,)),
        ],
        compiler_params=pltpu.CompilerParams(
            collective_id=0,
            disable_semaphore_checks=True,
        ),
    )(x)
```
